```python
import numpy as np

kernel_name = "dist_pipemlp_pp2tp2_xy_b4096_d256_h512"

def setup_inputs():
    x_padded = np.zeros((2, 4096, 256), dtype=np.float32)
    x_padded[0] = np.random.randn(4096, 256).astype(np.float32)
    Win = np.random.randn(4, 256, 1024).astype(np.float32)
    Wout = np.random.randn(4, 1024, 256).astype(np.float32)
    return {"x_padded": x_padded, "Win": Win, "Wout": Wout}

def reference(x_padded, Win, Wout):
    a = x_padded[0]
    for k in range(4):
        h = a @ Win[k]
        h = np.maximum(h, 0.0)
        a = h @ Wout[k]
    out = np.zeros_like(x_padded)
    out[1] = a
    return out
```

```python
import jax
import jax.numpy as jnp
from jax import lax
from jax.experimental import pallas as pl
from jax.experimental.pallas import tpu as pltpu

MESH = pl.DeviceIdType.MESH
BF16 = jnp.bfloat16
F32 = jnp.float32

HALF = 2048
CH = 128
HC = CH // 2
NCH = HALF // CH
BLOCK = 512
AHEAD = 12
DEFER = 4
EARLY_L2 = (8, 10, 12, 14)
FIRST = 48
EXTRA = 48

SENDS_DEFERRED = ((0, HC), (HC, HC), (CH, (DEFER - 1) * CH))
SENDS_STREAMED = (
    (4 * CH, 3 * CH, False, 6),
    (7 * CH, 2 * CH, False, 8),
    (9 * CH, CH, True, 9),
    (10 * CH, CH, True, 10),
    (11 * CH, CH, True, 11),
    (12 * CH, CH, False, 12),
    (13 * CH, CH, False, 13),
    (14 * CH, EXTRA, True, 14),
    (14 * CH + EXTRA, CH - EXTRA, False, 14),
    (15 * CH, CH, False, 15),
)


def _transfers():
    sends = [(r0, nr, False) for r0, nr in SENDS_DEFERRED] + [s[:3] for s in SENDS_STREAMED]
    sends = [(i,) + s for i, s in enumerate(sends)]
    near = [s for s in sends if not s[3]]
    far = [s for s in sends if s[3]]
    order, a, b, rows_a, rows_b = [], list(near), list(far), 0, 0
    while a or b:
        if a and (not b or rows_a <= rows_b):
            rows_a += a[-1][2]
            order.append(a.pop())
        else:
            rows_b += b[-1][2]
            order.append(b.pop())
    return sends, far, order[::-1]


def _body(x_hbm, win_hbm, wout_hbm, out,
          wi_f32, wo_f32, wi, wo, x_f32, p_send, p_recv, partial, a_send, a_recv,
          a3_buf, h_buf, f_send, f_recv,
          w_load_sem, x_load_sem, send_sem, w_sem, back_sem, row_sem, res_sem, ok_sem):
    mx, my = lax.axis_index("x"), lax.axis_index("y")
    ynbr, xnbr, diag = (mx, 1 - my), (1 - mx, my), (1 - mx, 1 - my)
    _, d, hid = wi.shape
    mine, theirs = my * HALF, (1 - my) * HALF
    sends, far_sends, arrivals = _transfers()

    pieces = ((0, 0, 0, FIRST), (0, 0, FIRST, d - FIRST), (0, 1, 0, hid), (1, 0, 0, d), (1, 1, 0, hid))
    first_layer, second_layer = (0, 1, 2), (3, 4)

    def w_load(i):
        slot, o, r0, nr = pieces[i]
        layer = (1 - mx) if slot == 0 else mx
        src, dst = ((win_hbm, wi_f32), (wout_hbm, wo_f32))[o]
        return pltpu.make_async_copy(
            src.at[layer, pl.ds(r0, nr)], dst.at[slot, pl.ds(r0, nr)], w_load_sem.at[i])

    def w_cast(i):
        slot, o, r0, nr = pieces[i]
        src, dst = ((wi_f32, wi), (wo_f32, wo))[o]
        dst[slot, pl.ds(r0, nr)] = src[slot, pl.ds(r0, nr)].astype(BF16)

    def remote(src, dst, ssem, rsem, dev):
        return pltpu.make_async_remote_copy(src, dst, ssem, rsem, device_id=dev, device_id_type=MESH)

    def w_swap(i):
        slot, o, r0, nr = pieces[i]
        buf = (wi, wo)[o]
        return remote(buf.at[slot, pl.ds(r0, nr)], buf.at[2 + slot, pl.ds(r0, nr)],
                      send_sem.at[0], w_sem.at[i], ynbr)

    def w_back(j, i):
        _, o, r0, nr = pieces[i]
        buf = (wi, wo)[o]
        return remote(buf.at[2 * j, pl.ds(r0, nr)], buf.at[3 + j, pl.ds(r0, nr)],
                      send_sem.at[1], back_sem.at[o], xnbr)

    def rows(start, size):
        return pl.ds(start if isinstance(start, int) else pl.multiple_of(start, 16), size)

    def p_copy(r0, nr):
        return remote(p_send.at[rows(r0, nr)], p_recv.at[rows(r0, nr)],
                      send_sem.at[2], row_sem.at[r0 // HC], ynbr)

    def a_copy(r0, nr):
        return remote(a_send.at[rows(r0, nr)], a_recv.at[rows(r0, nr)],
                      send_sem.at[3], row_sem.at[r0 // HC], xnbr)

    def f_copy(sem, r0, nr, dev):
        return remote(f_send.at[rows(r0, nr)], f_recv.at[rows(r0, nr)],
                      send_sem.at[2], res_sem.at[sem], dev)

    def f_forward(sem, r0, nr):
        return remote(f_recv.at[rows(r0, nr)], f_recv.at[rows(r0, nr)],
                      send_sem.at[1], res_sem.at[sem], xnbr)

    def x_theirs(j):
        return pltpu.make_async_copy(
            x_hbm.at[0, rows(theirs + j * BLOCK, BLOCK)], x_f32.at[rows(j * BLOCK, BLOCK)], x_load_sem.at[j])

    def x_mine():
        return pltpu.make_async_copy(
            x_hbm.at[0, rows(mine, HALF)], x_f32.at[rows(HALF, HALF)], x_load_sem.at[HALF // BLOCK])

    def wait_all(ref, sem):
        pltpu.make_async_copy(ref, ref, sem).wait()

    def signal(sem, dev):
        pl.semaphore_signal(sem, 1, device_id=dev, device_id_type=MESH)

    def hidden(v, slot):
        h = jnp.dot(v, wi[slot], preferred_element_type=F32)
        return jnp.maximum(h, 0.0).astype(BF16)

    def ffn(v, slot):
        return jnp.dot(hidden(v, slot), wo[slot], preferred_element_type=F32)

    def layer(v, s0, s1):
        return (ffn(v, s0) + ffn(v, s1)).astype(BF16)

    def loop(lo, hi, fn):
        def step(k, carry):
            fn(k)
            return carry
        lax.fori_loop(lo, hi, step, 0)

    def member(k, chunks):
        return (jnp.right_shift(sum(1 << c for c in chunks), k) & 1) == 1

    corner = jnp.logical_and(mx == 0, my == 0)
    bridge = jnp.logical_and(mx == 1, my == 0)
    barrier = pltpu.get_barrier_semaphore()
    w_load(0).start()
    signal(barrier, ynbr)
    pl.when(bridge)(lambda: signal(barrier, xnbr))
    for i in first_layer[1:]:
        w_load(i).start()

    w_load(0).wait()
    w_cast(0)
    pl.when(corner)(lambda: pl.semaphore_wait(barrier, 2))
    pl.when(jnp.logical_not(corner))(lambda: pl.semaphore_wait(barrier, 1))
    w_swap(0).start()
    for i in second_layer:
        w_load(i).start()
    pl.when(mx == 0)(x_theirs(0).start)
    pl.when(corner)(lambda: signal(ok_sem, xnbr))

    w_load(1).wait()
    w_cast(1)
    w_swap(1).start()

    @pl.when(mx == 1)
    def _():
        pl.semaphore_wait(ok_sem, 1)

        @pl.when(bridge)
        def _():
            signal(ok_sem, ynbr)
            signal(ok_sem, diag)

        w_back(0, 0).start()
        w_back(0, 1).start()

    w_load(2).wait()
    w_cast(2)
    w_swap(2).start()
    pl.when(mx == 1)(w_back(0, 2).start)

    @pl.when(mx == 0)
    def _():
        for j in range(1, HALF // BLOCK):
            x_theirs(j).start()
        x_mine().start()

    for i in second_layer:
        w_load(i).wait()
        w_cast(i)
        pl.when(mx == 1)(w_swap(i).start)

    @pl.when(mx == 0)
    def _stage0():
        def layer0_theirs(j):
            x_theirs(j).wait()
            p_send[rows(j * BLOCK, BLOCK)] = ffn(x_f32[rows(j * BLOCK, BLOCK)].astype(BF16), 1).astype(BF16)
            for i in range(BLOCK // CH):
                k = j * (BLOCK // CH) + i

                @pl.when(member(k, EARLY_L2))
                def _():
                    p_copy(k * CH, HC).start()
                    p_copy(k * CH + HC, HC).start()

                pl.when(jnp.logical_not(member(k, EARLY_L2)))(p_copy(k * CH, CH).start)

        def layer0_mine(r0, nr):
            partial[rows(r0, nr)] = ffn(x_f32[rows(HALF + r0, nr)].astype(BF16), 1)

        def stream(r0, nr, with_layer2):
            p_copy(r0, nr).wait_recv()
            a = (partial[rows(r0, nr)] + p_recv[rows(r0, nr)].astype(F32)).astype(BF16)
            a = layer(a, 0, 2)
            if with_layer2:
                a = layer(a, 3, 4)
            a_send[rows(r0, nr)] = a
            a_copy(r0, nr).start()

        def chunk(k):
            @pl.when(k == EARLY_L2[0])
            def _():
                wait_all(wi.at[pl.ds(3, 2)], back_sem.at[0])
                wait_all(wo.at[pl.ds(3, 2)], back_sem.at[1])

            pl.when(member(k, EARLY_L2))(lambda: loop(0, 2, lambda i: stream(k * CH + i * HC, HC, True)))
            pl.when(jnp.logical_not(member(k, EARLY_L2)))(lambda: stream(k * CH, CH, False))
            pl.when(k < NCH - AHEAD)(lambda: layer0_mine((k + AHEAD) * CH, CH))

        loop(0, HALF // BLOCK, layer0_theirs)
        x_mine().wait()
        loop(0, AHEAD * CH // BLOCK, lambda j: layer0_mine(j * BLOCK, BLOCK))
        pl.when(my == 1)(lambda: pl.semaphore_wait(ok_sem, 1))
        for i in first_layer:
            w_swap(i).wait_recv()
        loop(0, NCH, chunk)

        def clear(k):
            out[0, rows(k * 2 * CH, 2 * CH)] = jnp.zeros((2 * CH, d), F32)

        loop(0, NCH, clear)
        for sem, r0, nr, _ in far_sends:
            f_forward(sem, r0, nr).wait_recv()
            f_forward(sem, r0, nr).start()

        for i in first_layer:
            w_swap(i).wait_send()
        wait_all(p_send, send_sem.at[2])
        wait_all(a_send, send_sem.at[3])
        for sem, r0, nr, _ in far_sends:
            f_forward(sem, r0, nr).wait_send()

    @pl.when(mx == 1)
    def _stage1():
        def keep(r0, nr, res):
            f_send[rows(r0, nr)] = res
            out[0, rows(mine + r0, nr)] = res.astype(F32)

        def peer_hidden(k):
            h_buf[rows(k * CH, CH)] = hidden(a3_buf[rows(k * CH, CH)], 3)

        def early(k, behind=True):
            a_copy(k * CH, CH).wait_recv()
            a3 = layer(a_recv[rows(k * CH, CH)], 0, 2)
            if behind:
                peer_hidden(k - 1)
            a3_buf[rows(k * CH, CH)] = a3
            partial[rows(k * CH, CH)] = ffn(a3, 1)

        def late(sem, r0, nr):
            rest = jnp.dot(h_buf[rows(r0, nr)], wo[3], preferred_element_type=F32)
            keep(r0, nr, (partial[rows(r0, nr)] + rest).astype(BF16))
            f_copy(sem, r0, nr, ynbr).start()

        def both(k):
            a_copy(k * CH, CH).wait_recv()
            keep(k * CH, CH, layer(layer(a_recv[rows(k * CH, CH)], 0, 2), 1, 3))

        def last(k):
            @pl.when(k != DEFER)
            def _():
                a_copy(k * CH, HC).wait_recv()
                a_copy(k * CH + HC, HC).wait_recv()

            keep(k * CH, CH, layer(a_recv[rows(k * CH, CH)], 1, 3))

        def chunk(k):
            short = member(k, EARLY_L2 + (DEFER,))
            pl.when(short)(lambda: last(k))
            pl.when(jnp.logical_not(short))(lambda: both(k))
            for (sem, r0, nr, far), s in zip(sends[len(SENDS_DEFERRED):], SENDS_STREAMED):
                pl.when(k == s[3])(f_copy(sem, r0, nr, diag if far else ynbr).start)

        for i in first_layer:
            w_swap(i).wait_recv()
            w_back(1, i).start()
        early(0, behind=False)
        w_swap(second_layer[0]).wait_recv()
        loop(1, DEFER, early)
        a_copy(DEFER * CH, CH).wait_recv()
        a3 = layer(a_recv[rows(DEFER * CH, CH)], 0, 2)
        peer_hidden(DEFER - 1)
        a_recv[rows(DEFER * CH, CH)] = a3
        w_swap(second_layer[1]).wait_recv()
        for sem, r0, nr, _ in sends[:len(SENDS_DEFERRED)]:
            late(sem, r0, nr)
        loop(DEFER, NCH, chunk)

        for i in first_layer + second_layer:
            w_swap(i).wait_send()
        for j in range(2):
            for i in first_layer:
                w_back(j, i).wait_send()
        for sem, r0, nr, _ in arrivals:
            f_copy(sem, r0, nr, ynbr).wait_recv()
            out[0, rows(theirs + r0, nr)] = f_recv[rows(r0, nr)].astype(F32)
        wait_all(f_send, send_sem.at[2])


def pallas_dist_pipemlp_pp2tp2_xy_b4096_d256_h512_kernel(
    x_padded: jax.Array,
    Win: jax.Array,
    Wout: jax.Array,
):
    _, batch, d = x_padded.shape
    hid = Win.shape[2]
    assert batch == 2 * HALF
    dma = pltpu.SemaphoreType.DMA
    act = pltpu.VMEM((HALF, d), BF16)
    return pl.pallas_call(
        _body,
        out_shape=jax.ShapeDtypeStruct(x_padded.shape, x_padded.dtype),
        in_specs=[pl.BlockSpec(memory_space=pltpu.HBM)] * 3,
        out_specs=pl.BlockSpec(memory_space=pltpu.VMEM),
        scratch_shapes=[
            pltpu.VMEM((2, d, hid), F32), pltpu.VMEM((2, hid, d), F32),
            pltpu.VMEM((5, d, hid), BF16), pltpu.VMEM((5, hid, d), BF16),
            pltpu.VMEM((batch, d), F32),
            act, act, pltpu.VMEM((HALF, d), F32), act, act,
            pltpu.VMEM((DEFER * CH, d), BF16), pltpu.VMEM((DEFER * CH, hid), BF16), act, act,
            dma((5,)), dma((HALF // BLOCK + 1,)), dma((4,)), dma((5,)), dma((2,)),
            dma((2 * NCH,)), dma((len(SENDS_DEFERRED) + len(SENDS_STREAMED),)),
            pltpu.SemaphoreType.REGULAR,
        ],
        compiler_params=pltpu.CompilerParams(
            collective_id=0,
            vmem_limit_bytes=48 * 2**20,
            disable_semaphore_checks=True,
        ),
    )(x_padded, Win, Wout)
```
